```python
import numpy as np

kernel_name = "dist_f_of_ar_i_m4096_n1024"

def setup_inputs():
    t = np.random.randn(16384, 1024).astype(np.float32)
    return {"t": t}

def reference(t: np.ndarray) -> np.ndarray:
    s = t.reshape(4, 4096, 1024).sum(axis=0)
    r = np.maximum(s, 0.0)
    return np.tanh(s) * s * s + r * r * r
```

```python
import jax
import jax.numpy as jnp
from jax import lax
from jax.experimental import pallas as pl
from jax.experimental.pallas import tpu as pltpu

M, N = 4096, 1024
Q = M // 8
MESH = pl.DeviceIdType.MESH
UP = ((0, 16), (16, 48), (64, 144), (208, 304))
MID = ((0, 256), (256, 256))
TILE = 32


def _rows_loop(off, size, fn):
    t = TILE if size % TILE == 0 else 16
    n = size // t
    if n <= 3:
        for i in range(n):
            fn(off + i * t, t)
    else:
        def it(i, c):
            fn(pl.multiple_of(off + i * t, 16), t)
            return c
        lax.fori_loop(0, n, it, 0)


def _kernel(x_hbm, out, xf, s1, r1, s2, r2, lsem, ssem, rsem):
    me = lax.axis_index("i")
    first = (me ^ 1, me ^ 3)
    second = (me ^ 3, me ^ 1)
    bar = pltpu.get_barrier_semaphore()
    for nb in first:
        pl.semaphore_signal(bar, inc=1, device_id=(nb,), device_id_type=MESH)

    px = me >> 1
    py = (me ^ px) & 1
    pos = (2 * py + px, 2 * px + py)
    OWN, SECOND, FIRST, DIAG = 0, 1, 2, 3

    def rows(h, role, off, size):
        return pl.ds(pl.multiple_of((h * 4 + (pos[h] ^ role)) * Q + off, 16), size)

    def load(role, off, size, sem):
        return [
            pltpu.make_async_copy(
                x_hbm.at[rows(h, role, off, size)],
                xf.at[role, h, pl.ds(off, size)],
                lsem.at[sem],
            )
            for h in (0, 1)
        ]

    def remote(src, dst, sem, dev):
        return pltpu.make_async_remote_copy(
            src, dst, ssem, rsem.at[sem], device_id=(dev,), device_id_type=MESH
        )

    def gather(h, role, off, size, sem, dev):
        blk = out.at[rows(h, role, off, size)]
        return remote(blk, blk, sem, dev)

    def arrived(buf, sem):
        pltpu.make_async_copy(buf, buf, rsem.at[sem]).wait()

    H = (0, 1)
    nu, nm = len(UP), len(MID)
    ld_diag = [load(DIAG, o, s, k) for k, (o, s) in enumerate(UP)]
    ld_first = load(FIRST, 0, Q, nu)
    ld_late = load(SECOND, 0, Q, nu + 1) + load(OWN, 0, Q, nu + 1)

    R1A, R1B, R2, R3, R4 = 0, 1, 2, 2 + nm, 4 + nm
    p1a = [[remote(s1.at[0, h, pl.ds(o, s)], r1.at[0, h, pl.ds(o, s)], R1A, first[h]) for h in H] for o, s in UP]
    p1b = [remote(s1.at[1, h], r1.at[1, h], R1B, first[h]) for h in H]
    p2 = [[remote(s2[k].at[h], r2[k].at[h], R2 + k, second[h]) for h in H] for k in range(nm)]
    p3 = [[gather(h, OWN, o, s, R3 + h, second[h]) for h in H] for o, s in MID]
    p4a = [gather(h, OWN, 0, Q, R4 + h, first[h]) for h in H]
    p4b = [gather(h, SECOND, 0, Q, R4 + h, first[h]) for h in H]

    for pair in ld_diag:
        for c in pair:
            c.start()

    def to_bf16(h, role, slot, off, size):
        def fn(o, t):
            r = pl.ds(o, t)
            s1[slot, h, r, :] = xf[role, h, r, :].astype(jnp.bfloat16)
        _rows_loop(off, size, fn)

    for k, (o, s) in enumerate(UP):
        for c in ld_diag[k]:
            c.wait()
        for h in H:
            to_bf16(h, DIAG, 0, o, s)
        if k == 0:
            pl.semaphore_wait(bar, 2)
        for h in H:
            p1a[k][h].start()
        if k == 0:
            for c in ld_first:
                c.start()
    for c in ld_late:
        c.start()
    for c in ld_first:
        c.wait()
    for h in H:
        to_bf16(h, FIRST, 1, 0, Q)
        p1b[h].start()

    for c in ld_late:
        c.wait()
    arrived(r1.at[0], R1A)
    for k, (o, s) in enumerate(MID):
        for h in H:
            def fn(i, t, h=h, k=k, o=o):
                r = pl.ds(o + i, t)
                s2[k][h, pl.ds(i, t), :] = (
                    xf[SECOND, h, r, :] + r1[0, h, r, :].astype(jnp.float32)
                ).astype(jnp.bfloat16)
            _rows_loop(0, s, fn)
            p2[k][h].start()

    arrived(r1.at[1], R1B)
    for k, (o, s) in enumerate(MID):
        arrived(r2[k], R2 + k)
        for h in H:
            def fn(i, t, h=h, k=k, o=o):
                r = pl.ds(o + i, t)
                v = xf[OWN, h, r, :] + r1[1, h, r, :].astype(jnp.float32)
                v = v + r2[k][h, pl.ds(i, t), :].astype(jnp.float32)
                p = jnp.maximum(v, 0.0)
                out[rows(h, OWN, o + i, t), :] = (jnp.tanh(v) * v * v + p * p * p).astype(jnp.bfloat16)
            _rows_loop(0, s, fn)
            p3[k][h].start()
    for h in H:
        p4a[h].start()
    for h in H:
        arrived(out.at[rows(h, SECOND, 0, Q)], R3 + h)
        p4b[h].start()
    for c in [c for pair in p1a + p2 + p3 for c in pair] + p1b + p4a + p4b:
        c.wait_send()
    for h in H:
        far = pl.multiple_of((h * 4 + ((pos[h] ^ FIRST) & 2)) * Q, Q)
        arrived(out.at[pl.ds(far, 2 * Q)], R4 + h)


def pallas_dist_f_of_ar_i_m4096_n1024_kernel(
t: jax.Array,
):
    return pl.pallas_call(
        _kernel,
        out_shape=pltpu.VMEM((M, N), jnp.bfloat16),
        in_specs=[pl.BlockSpec(memory_space=pltpu.HBM)],
        out_specs=pl.BlockSpec(memory_space=pltpu.VMEM),
        scratch_shapes=[
            pltpu.VMEM((4, 2, Q, N), jnp.float32),
            pltpu.VMEM((2, 2, Q, N), jnp.bfloat16),
            pltpu.VMEM((2, 2, Q, N), jnp.bfloat16),
            [pltpu.VMEM((2, s, N), jnp.bfloat16) for _, s in MID],
            [pltpu.VMEM((2, s, N), jnp.bfloat16) for _, s in MID],
            pltpu.SemaphoreType.DMA((len(UP) + 2,)),
            pltpu.SemaphoreType.DMA,
            pltpu.SemaphoreType.DMA((len(MID) + 6,)),
        ],
        compiler_params=pltpu.CompilerParams(
            collective_id=0,
            vmem_limit_bytes=48 * 2**20,
        ),
    )(t)
```

```python
import jax
import jax.numpy as jnp
from jax import lax
from jax.experimental import pallas as pl
from jax.experimental.pallas import tpu as pltpu

M, N = 4096, 1024
Q = M // 8
HALF = Q // 2
DETOUR = 16
BODY = Q - DETOUR
RAMP = ((0, 8), (8, 16), (24, 32), (56, 64), (120, 128), (248, BODY - 248))
TO_CHIP2_AT = 1
DETOUR_AT = 3
LOADS_AHEAD = 2
TILE = 32

HALVES = (0, 1)
OWN, SECOND, FIRST, DIAG = 0, 1, 2, 3
R1A, R1B, R2, R3, R4, RDETOUR, N_RECV = 0, 1, 2, 4, 6, 8, 9
MESH = pl.DeviceIdType.MESH


def _for_rows(off, size, fn):
    n = size // TILE
    if n <= 2:
        for i in range(n):
            fn(off + i * TILE, TILE)
    else:

        @pl.loop(0, n)
        def _(i):
            fn(pl.multiple_of(off + i * TILE, 8), TILE)

    if size % TILE:
        fn(off + n * TILE, size % TILE)


def _kernel(x_hbm, out, x, s1, r1, rd, s2, r2, load_sem, send_sem, recv_sem, ready):
    me = lax.axis_index("i")
    first = (me ^ 1, me ^ 3)
    second = (me ^ 3, me ^ 1)
    px = me >> 1
    py = (me ^ px) & 1
    pos = (2 * py + px, 2 * px + py)
    barrier = pltpu.get_barrier_semaphore()

    def signal_neighbours(sem):
        for dev in first:
            pl.semaphore_signal(sem, inc=1, device_id=(dev,), device_id_type=MESH)

    def rows(h, whose, off, size):
        start = (4 * h + (pos[h] ^ whose)) * Q + off
        return pl.ds(pl.multiple_of(start, 8), size)

    def remote(src, dst, sem, dev):
        return pltpu.make_async_remote_copy(
            src, dst, send_sem, recv_sem.at[sem],
            device_id=(dev,), device_id_type=MESH,
        )

    def gather(h, whose, off, size, sem, dev):
        block = out.at[rows(h, whose, off, size)]
        return remote(block, block, sem, dev)

    def arrived(buf, sem):
        pltpu.make_async_copy(buf, buf, recv_sem.at[sem]).wait()

    groups = [[(DIAG, off, size)] for off, size in RAMP]
    groups[DETOUR_AT].append((DIAG, BODY, DETOUR))
    groups += [[(FIRST, 0, Q)], [(SECOND, 0, Q), (OWN, 0, Q)]]
    loads = [
        [
            pltpu.make_async_copy(
                x_hbm.at[rows(h, whose, off, size)],
                x.at[whose, h, pl.ds(off, size)],
                load_sem.at[g % (LOADS_AHEAD + 1)],
            )
            for whose, off, size in group
            for h in HALVES
        ]
        for g, group in enumerate(groups)
    ]

    tail = pl.ds(BODY, DETOUR)
    p1a = [
        [
            remote(s1.at[0, h, pl.ds(off, size)], r1.at[0, h, pl.ds(off, size)], R1A, first[h])
            for h in HALVES
        ]
        for off, size in RAMP
    ]
    p1a_tail = [remote(s1.at[0, h, tail], r1.at[0, h, tail], R1A, first[h]) for h in HALVES]
    p1a_detour = [remote(s1.at[0, h, tail], rd.at[h], RDETOUR, 2) for h in HALVES]
    p1b = [remote(s1.at[1, h], r1.at[1, h], R1B, first[h]) for h in HALVES]
    p2 = [
        [remote(s2.at[h, pl.ds(k * HALF, HALF)], r2.at[k, h], R2 + k, second[h]) for h in HALVES]
        for k in range(2)
    ]
    p3 = [
        [gather(h, OWN, k * HALF, HALF, R3 + h, second[h]) for h in HALVES]
        for k in range(2)
    ]
    p4a = [gather(h, OWN, 0, Q, R4 + h, first[h]) for h in HALVES]
    p4b = [gather(h, SECOND, 0, Q, R4 + h, first[h]) for h in HALVES]

    @pl.when(me != 2)
    def _():
        signal_neighbours(barrier)

    for group in loads[:LOADS_AHEAD]:
        for copy in group:
            copy.start()

    @pl.when((me & 1) == 1)
    def _():
        pl.semaphore_wait(barrier, 1)

    @pl.when((me & 1) == 0)
    def _():
        pl.semaphore_wait(barrier, 2)

    @pl.when(me == 2)
    def _():
        signal_neighbours(ready)

    def pack(h, whose, slot, off, size):
        def tile(i, t):
            r = pl.ds(i, t)
            s1[slot, h, r, :] = x[whose, h, r, :].astype(jnp.bfloat16)

        _for_rows(off, size, tile)

    for k, (off, size) in enumerate(RAMP):
        for copy in loads[k]:
            copy.wait()
        for h in HALVES:
            pack(h, DIAG, 0, off, size)
        if k > TO_CHIP2_AT:
            for h in HALVES:
                p1a[k][h].start()
        else:
            for h in HALVES:

                @pl.when(first[h] != 2)
                def _():
                    p1a[k][h].start()

        if k == TO_CHIP2_AT:
            for h in HALVES:

                @pl.when(first[h] == 2)
                def _():
                    pl.semaphore_wait(ready, 1)
                    for chunk in p1a[: k + 1]:
                        chunk[h].start()

        if k == DETOUR_AT:
            for h in HALVES:
                pack(h, DIAG, 0, BODY, DETOUR)

                @pl.when(first[h] != 0)
                def _():
                    p1a_tail[h].start()

                @pl.when(first[h] == 0)
                def _():
                    p1a_detour[h].start()

        for copy in loads[k + LOADS_AHEAD]:
            copy.start()

    for copy in loads[len(RAMP)]:
        copy.wait()

    @pl.when(me == 2)
    def _():
        arrived(rd, RDETOUR)
        for h in HALVES:
            x[FIRST, h, tail, :] += rd[h].astype(jnp.float32)

    for h in HALVES:
        pack(h, FIRST, 1, 0, Q)
        p1b[h].start()

    for copy in loads[len(RAMP) + 1]:
        copy.wait()

    @pl.when(me == 0)
    def _():
        for h in HALVES:
            r1[0, h, tail, :] = jnp.zeros((DETOUR, N), jnp.bfloat16)
        arrived(r1.at[0, :, pl.ds(0, BODY)], R1A)

    @pl.when(me != 0)
    def _():
        arrived(r1.at[0], R1A)

    for h in HALVES:

        def pair_sum(i, t, h=h):
            r = pl.ds(i, t)
            s = x[SECOND, h, r, :] + r1[0, h, r, :].astype(jnp.float32)
            s2[h, r, :] = s.astype(jnp.bfloat16)

        _for_rows(0, Q, pair_sum)
        for k in range(2):
            p2[k][h].start()

    arrived(r1.at[1], R1B)
    for k in range(2):
        arrived(r2.at[k], R2 + k)
        for h in HALVES:

            def finish(i, t, h=h, k=k):
                r = pl.ds(k * HALF + i, t)
                s = x[OWN, h, r, :] + r1[1, h, r, :].astype(jnp.float32)
                s = s + r2[k, h, pl.ds(i, t), :].astype(jnp.float32)
                relu = jnp.maximum(s, 0.0)
                y = jnp.tanh(s) * s * s + relu * relu * relu
                out[rows(h, OWN, k * HALF + i, t), :] = y.astype(out.dtype)

            _for_rows(0, HALF, finish)
            p3[k][h].start()

    for h in HALVES:
        p4a[h].start()
    for h in HALVES:
        arrived(out.at[rows(h, SECOND, 0, Q)], R3 + h)
        p4b[h].start()

    for step in (*p1a, p1a_tail, p1b, *p2, *p3, p4a, p4b):
        for copy in step:
            copy.wait_send()
    for h in HALVES:
        start = (4 * h + ((pos[h] ^ FIRST) & 2)) * Q
        arrived(out.at[pl.ds(pl.multiple_of(start, Q), 2 * Q)], R4 + h)


def pallas_dist_f_of_ar_i_m4096_n1024_kernel(
t: jax.Array,
):
    return pl.pallas_call(
        _kernel,
        out_shape=jax.ShapeDtypeStruct((M, N), jnp.bfloat16),
        in_specs=[pl.BlockSpec(memory_space=pltpu.HBM)],
        out_specs=pl.BlockSpec(memory_space=pltpu.VMEM),
        scratch_shapes=[
            pltpu.VMEM((4, 2, Q, N), jnp.float32),
            pltpu.VMEM((2, 2, Q, N), jnp.bfloat16),
            pltpu.VMEM((2, 2, Q, N), jnp.bfloat16),
            pltpu.VMEM((2, DETOUR, N), jnp.bfloat16),
            pltpu.VMEM((2, Q, N), jnp.bfloat16),
            pltpu.VMEM((2, 2, HALF, N), jnp.bfloat16),
            pltpu.SemaphoreType.DMA((LOADS_AHEAD + 1,)),
            pltpu.SemaphoreType.DMA,
            pltpu.SemaphoreType.DMA((N_RECV,)),
            pltpu.SemaphoreType.REGULAR,
        ],
        compiler_params=pltpu.CompilerParams(
            collective_id=0,
            vmem_limit_bytes=48 * 2**20,
        ),
    )(t)
```
